```python
import numpy as np

kernel_name = "dist_sparse_attn_strided_qseq_kvseq_b2_sq128_skv128_hq4_dh64"

def setup_inputs():
    x = np.random.randn(2, 512, 512).astype(np.float32)
    Wq = np.random.randn(512, 256).astype(np.float32) * 0.02
    K_ext = np.random.randn(2, 512, 4, 64).astype(np.float32)
    V_ext = np.random.randn(2, 512, 4, 64).astype(np.float32)
    Wo = np.random.randn(256, 512).astype(np.float32) * 0.02
    return {"x": x, "Wq": Wq, "K_ext": K_ext, "V_ext": V_ext, "Wo": Wo}

def reference(x, Wq, K_ext, V_ext, Wo):
    B, Sq, Skv, Hq, Dh = 2, 512, 512, 4, 64
    Q = (x @ Wq).reshape(B, Sq, Hq, Dh)
    qb = (np.arange(Sq) // 64)[:, None]
    kb = (np.arange(Skv) // 64)[None, :]
    mask = (qb == kb) | ((kb % 4) == (qb % 4))
    scores = np.einsum('bihd,bjhd->bhij', Q, K_ext).astype(np.float32) * 0.125
    scores = np.where(mask[None, None, :, :], scores, -1e9)
    scores_max = scores.max(axis=-1, keepdims=True)
    w = np.exp(scores - scores_max)
    row_keep = mask.any(axis=1)
    w_sum = np.where(row_keep[None, None, :, None], w.sum(axis=-1, keepdims=True), 1.0)
    w = w / w_sum
    w = np.where(row_keep[None, None, :, None], w, 0.0)
    ctx = np.einsum('bhij,bjhd->bihd', w, V_ext).reshape(B, Sq, Hq * Dh)
    return ctx @ Wo
```

```python
import jax
import jax.numpy as jnp
from jax import lax
from jax.experimental import pallas as pl
from jax.experimental.pallas import tpu as pltpu

B, S, DM, H, DH = 2, 128, 512, 4, 64
HD = H * DH
BLK = 64
F32, BF16, U32 = jnp.float32, jnp.bfloat16, jnp.uint32
MESH = pl.DeviceIdType.MESH
NT = (((1,), (1,)), ((), ()))
QSCALE = 0.125 * 1.4426950408889634

NCH = 8
LAST = NCH - 1
NRL = NCH + 1
CR = 32
HEAD = 20
H16 = 16
NPC = (DH - H16) // 16
KEEP = 20


def _pack(x):
    return pltpu.bitcast(x.astype(BF16), U32)


def _unpack(w):
    return pltpu.bitcast(w, BF16)


def _body(x_hbm, wq_hbm, kt_hbm, vt_hbm, wo_hbm, out_ref,
          xf, wqf, kf, vf, wof, loc, rem, rl, wqb, wob, qb, sl, p_loc, p_rem, inv_l,
          hx, qx, px, inv_x, cx,
          ld_sem, own_sem, head_sem, fw_sem, fw2_sem, rl_sem, fin_sem, hx_sem, qx_sem, rdy_sem):
    me = lax.axis_index("i")
    odd = me & 1
    nbr = (1 - odd, 3 - odd)
    side = me >> 1
    is0, is2, is_odd = me == 0, me == 2, odd == 1

    def signal(sem, dev):
        pl.semaphore_signal(sem, inc=1, device_id=(dev,), device_id_type=MESH)

    def rdma(src, dst, send_sem, recv_sem, dev):
        return pltpu.make_async_remote_copy(src, dst, send_sem, recv_sem,
                                            device_id=(dev,), device_id_type=MESH)

    bar = pltpu.get_barrier_semaphore()

    @pl.when(me != 2)
    def _():
        signal(bar, nbr[0])
        signal(bar, nbr[1])

    def head_send(p):
        return rdma(kt_hbm.at[pl.ds(p * 128, HEAD)], hx.at[side],
                    head_sem.at[p], hx_sem.at[side], nbr[p])

    @pl.when(is_odd)
    def _():
        pl.semaphore_wait(bar, 1)
        head_send(0).start()

    loads = []

    def load(src, dst):
        loads.append(pltpu.make_async_copy(src, dst, ld_sem.at[len(loads)]))
        return loads[-1]

    def load_rows(src, dst, r0, n):
        return load(src.at[pl.ds(r0, n)], dst.at[pl.ds(r0, n)])

    k0_tail = [[load_rows(kt_hbm, kf, p * 128 + H16 + 16 * j, 16) for p in range(2)]
               for j in range(NPC)]
    k0_b = [load_rows(kt_hbm, kf, p * 128 + DH, DH) for p in range(2)]
    k1 = [load_rows(kt_hbm, kf, HD + p * 128, 128) for p in range(2)]
    n_urgent = len(loads)
    k0_head = [load_rows(kt_hbm, kf, p * 128, H16) for p in range(2)]
    v_ld = [[load_rows(vt_hbm, vf, b * HD + p * 128, 128) for b in range(B)] for p in range(2)]
    wq_ld = load(wq_hbm, wqf)
    x_ld = {b: load(x_hbm.at[b], xf.at[b]) for b in (1, 0)}
    wo_ld = load(wo_hbm, wof)

    for cp in loads[:n_urgent]:
        cp.start()

    @pl.when(is2)
    def _():
        pl.semaphore_wait(bar, 2)
        head_send(0).start()
        head_send(1).start()
        signal(rdy_sem, nbr[0])
        signal(rdy_sem, nbr[1])

    for cp in loads[n_urgent:]:
        cp.start()

    def own_send(c, p, via=None, slot=None, r0=0, n=CR):
        via = p if via is None else via
        slot = side * NRL + (c if slot is None else slot)
        rdma(loc.at[p * NCH + c, pl.ds(r0, n)], rl.at[slot, pl.ds(r0, n)],
             own_sem, rl_sem.at[slot], nbr[via]).start()

    def rl_wait(slot, s, r0=0, n=CR):
        ref = rl.at[s * NRL + slot, pl.ds(r0, n)]
        rdma(ref, ref, own_sem, rl_sem.at[s * NRL + slot], nbr[s]).wait_recv()

    def fwd(slot, s, dst=None, r0=0, n=CR):
        dst = side * NCH + slot if dst is None else dst
        rdma(rl.at[s * NRL + slot, pl.ds(r0, n)], rem.at[dst, pl.ds(r0, n)],
             fw_sem if n == CR else fw2_sem, fin_sem.at[dst], nbr[1 - s]).start()

    def relay(slot, s, dst=None, r0=0, n=CR):
        rl_wait(slot, s, r0, n)
        fwd(slot, s, dst, r0, n)

    def fin_wait(c, p):
        ref = rem.at[p * NCH + c]
        rdma(ref, ref, own_sem, fin_sem.at[p * NCH + c], nbr[p]).wait_recv()

    def sent(sem, ref):
        rdma(ref, ref, sem, rl_sem.at[0], nbr[0]).wait_send()

    lo32 = lax.broadcasted_iota(jnp.int32, (CR, 128), 1) < BLK
    lo64 = lax.broadcasted_iota(jnp.int32, (BLK, 128), 1) < BLK
    row128 = lax.broadcasted_iota(jnp.int32, (128, 128), 0)
    col128 = lax.broadcasted_iota(jnp.int32, (128, 128), 1)

    def swap(t):
        return pltpu.roll(t, BLK, 1)

    def blocks(top, bot, flip=False):
        z = jnp.zeros_like(top)
        if flip:
            parts = [jnp.where(lo32, z, top), jnp.where(lo32, bot, z)]
        else:
            parts = [jnp.where(lo32, top, z), jnp.where(lo32, z, bot)]
        return _unpack(jnp.concatenate(parts, axis=0))

    def uid(b, blk, p):
        return (b * 2 + blk) * 2 + p

    def flipped(b, blk):
        return b == 0 and blk == 1

    def mm(a, w):
        return jnp.dot(a, w, preferred_element_type=F32)

    early = (me != 0, is2)

    for j in range(NPC):
        for p in range(2):
            k0_tail[j][p].wait()
            r0 = H16 // 2 + 8 * j
            loc[p * NCH, r0:r0 + 8, :] = _pack(kf[p * 128 + 2 * r0:p * 128 + 2 * r0 + 16, :])
            s0 = max(r0, HEAD // 2)
            pl.when(early[p])(lambda: own_send(0, p, r0=s0, n=r0 + 8 - s0))

    for p in range(2):
        k0_b[p].wait()
        loc[p * NCH + 1] = _pack(kf[p * 128 + DH:(p + 1) * 128, :])
        pl.when(early[p])(lambda: own_send(1, p))

    for p in range(2):
        k1[p].wait()
        r = HD + p * 128
        a, b_ = _pack(kf[r:r + DH, :]), _pack(kf[r + DH:r + 128, :])
        cross = swap(jnp.where(lo32, b_, a))
        loc[p * NCH + 2] = jnp.where(lo32, a, cross)
        loc[p * NCH + 3] = jnp.where(lo32, cross, b_)

        @pl.when(early[p])
        def _():
            own_send(2, p)
            own_send(3, p)

    def prep_v(p):
        for b in range(B):
            v_ld[p][b].wait()
        eye = jnp.where(row128 == col128, 1.0, 0.0).astype(BF16)
        for b in range(B):
            r = b * HD + p * 128
            v = lax.dot_general(eye, vf[r:r + 128, :].astype(BF16), NT, preferred_element_type=F32)
            for blk in range(2):
                loc[p * NCH + 4 + 2 * b + blk] = _pack(v[blk * BLK:(blk + 1) * BLK])

    for p in range(2):
        k0_head[p].wait()
        loc[p * NCH, 0:H16 // 2, :] = _pack(kf[p * 128:p * 128 + H16, :])
    prep_v(0)

    @pl.when(me != 0)
    def _():
        for c in range(4, LAST):
            own_send(c, 0)

    pl.when(is2)(lambda: own_send(LAST, 0))
    pl.when(is_odd)(lambda: own_send(LAST, 0, n=KEEP))

    @pl.when(is0)
    def _():
        pl.semaphore_wait(bar, 2)
        for c in range(4):
            own_send(c, 0)
            own_send(c, 1)

    @pl.when(is_odd)
    def _():
        pl.semaphore_wait(rdy_sem, 1)
        for c in range(4):
            own_send(c, 1)

    prep_v(1)

    @pl.when(me != 0)
    def _():
        for c in range(4, NCH):
            own_send(c, 1)

    pl.when(is_odd)(lambda: own_send(LAST, 0, via=1, slot=NCH, r0=KEEP, n=CR - KEEP))

    def q_proj(b):
        x_ld[b].wait()
        q = mm(xf[b].astype(BF16), _unpack(wqb[...])) * QSCALE
        for blk in range(2):
            for p in range(2):
                qb[uid(b, blk, p)] = q[blk * BLK:(blk + 1) * BLK, p * 128:(p + 1) * 128].astype(BF16)

    def k_tile(buf, b, blk, p, swapped=True):
        c = p * NCH + 2 * b
        if b == 1:
            return blocks(buf[c + blk], buf[c + blk])
        return blocks(buf[c], buf[c + 1] if swapped else swap(buf[c + 1]), flipped(b, blk))

    def softmax(items):
        neg = jnp.float32(-jnp.inf)
        es = []
        for get_a, s_b, _ in items:
            mx = jnp.maximum(get_a(), s_b)
            m0 = jnp.max(jnp.where(lo64, mx, neg), axis=-1, keepdims=True)
            m1 = jnp.max(jnp.where(lo64, neg, mx), axis=-1, keepdims=True)
            m = jnp.where(lo64, m0, m1)
            es.append((jnp.exp2(get_a() - m), jnp.exp2(s_b - m)))
        res = []
        for (e_a, e_b), (_, _, flip) in zip(es, items):
            same = (row128 < BLK) == (col128 < BLK)
            ones = jnp.where(same != flip, 1.0, 0.0).astype(BF16)
            l = mm((e_a + e_b).astype(BF16), ones)
            r = pl.reciprocal(l, approx=True)
            res.append((e_a.astype(BF16), e_b.astype(BF16), r * (2.0 - l * r)))
        return res

    def context(p_a, v_a, p_b, v_b, inv, flip=False):
        return (mm(p_a, blocks(v_a, v_a, flip)) + mm(p_b, blocks(v_b, v_b, flip))) * inv

    wq_ld.wait()
    wqb[...] = _pack(wqf[...])
    q_proj(1)

    @pl.when(is0)
    def _():
        for p in range(2):
            rdma(qb.at[uid(1, 1, p)], qx, own_sem, qx_sem, nbr[p]).start()
        for c in (LAST, 4, 5, 6):
            own_send(c, 0)
            own_send(c, 1)

    headed = (is0, me != 2)
    for s in (1, 0):
        @pl.when(headed[s])
        def _():
            rdma(hx.at[s], hx.at[s], own_sem, hx_sem.at[s], nbr[s]).wait_recv()
            rl_wait(0, s, HEAD // 2, CR - HEAD // 2)
            h = _pack(jnp.concatenate([hx[s], jnp.zeros((2 * H16 - HEAD, 128), F32)], axis=0))
            top = lax.broadcasted_iota(jnp.int32, (H16, 128), 0) < HEAD // 2
            rl[s * NRL, 0:H16, :] = jnp.where(top, h, rl[s * NRL, 0:H16, :])

        pl.when(jnp.logical_not(headed[s]))(lambda: rl_wait(0, s))
        fwd(0, s)

    for s in range(2):
        rl_wait(1, s)
    for s in range(2):
        rl[s * NRL + 1] = swap(rl[s * NRL + 1])
    for s in (1, 0):
        fwd(1, s)

    q_proj(0)
    relay(2, 1)
    relay(2, 0)
    for b in range(B):
        for p in range(2):
            for blk in range(2):
                sl[uid(b, blk, p)] = mm(qb[uid(b, blk, p)], k_tile(loc, b, blk, p, swapped=False))
    wo_ld.wait()
    wob[...] = _pack(wof[...])

    @pl.when(odd == 0)
    def _():
        for slot in range(3, LAST):
            relay(slot, 0)
            relay(slot, 1)

    @pl.when(is0)
    def _():
        relay(LAST, 0, n=KEEP)
        relay(LAST, 1, n=KEEP)

    @pl.when(is2)
    def _():
        relay(LAST, 0)
        relay(LAST, 1)
        relay(NCH, 0, dst=LAST, r0=KEEP, n=CR - KEEP)
        relay(NCH, 1, dst=LAST, r0=KEEP, n=CR - KEEP)

    @pl.when(is_odd)
    def _():
        relay(3, 0)
        rl_wait(3, 1)
        relay(4, 1)
        rdma(qx, qx, own_sem, qx_sem, nbr[0]).wait_recv()
        s_a = mm(qx[...], blocks(rl[3], rl[3]))
        s_b = mm(qx[...], blocks(rl[NRL + 3], rl[NRL + 3]))
        (px[0], px[1], inv_x[...]), = softmax([(lambda: s_a, s_b, False)])
        relay(5, 1)
        rl_wait(LAST, 0)
        relay(4, 0)
        relay(6, 1)
        relay(5, 0)
        rl_wait(LAST, 1)
        cx[...] = _pack(context(px[0], rl[LAST], px[1], rl[NRL + LAST], inv_x[...]))
        dst = side * NCH + LAST
        rdma(cx, rem.at[dst], fw_sem, fin_sem.at[dst], nbr[0]).start()
        relay(6, 0)
        fwd(LAST, 0)

    def scores(b, blks):
        units = [(blk, p) for blk in blks for p in range(2)]
        for blk, p in units:
            fin_wait(2 * b + blk, p)
        s_rem = [mm(qb[uid(b, blk, p)], k_tile(rem, b, blk, p)) for blk, p in units]
        res = softmax([(lambda u=uid(b, blk, p): sl[u], s, flipped(b, blk))
                       for (blk, p), s in zip(units, s_rem)])
        for (blk, p), r in zip(units, res):
            u = uid(b, blk, p)
            p_loc[u], p_rem[u], inv_l[u] = r

    scores(0, (0, 1))
    pl.when(is0)(lambda: scores(1, (0,)))
    pl.when(me != 0)(lambda: scores(1, (0, 1)))

    def project(b, blk, ctx):
        out_ref[b, blk * BLK:(blk + 1) * BLK, :] = (
            mm(ctx[0], _unpack(wob[0:DH, :])) + mm(ctx[1], _unpack(wob[DH:2 * DH, :])))

    def own_context(b, blk):
        res = []
        for p in range(2):
            u, c = uid(b, blk, p), p * NCH + 4 + 2 * b + blk
            res.append(context(p_loc[u], loc[c], p_rem[u], rem[c], inv_l[u],
                               flipped(b, blk)).astype(BF16))
        return res

    for c in range(4, LAST):
        fin_wait(c, 0)
        fin_wait(c, 1)
        project((c - 4) // 2, c % 2, own_context((c - 4) // 2, c % 2))

    @pl.when(is2)
    def _():
        sent(own_sem, kf.at[pl.ds(0, 2 * NCH * CR - HEAD)])
        head_send(0).wait_send()
        head_send(1).wait_send()
        sent(fw_sem, kf.at[pl.ds(0, 2 * NCH * CR)])
        sent(fw2_sem, kf.at[pl.ds(0, 2 * (CR - KEEP))])

    @pl.when(is_odd)
    def _():
        sent(own_sem, kf.at[pl.ds(0, 2 * NCH * CR - HEAD // 2)])
        head_send(0).wait_send()
        sent(fw_sem, kf.at[pl.ds(0, (2 * NCH - 1) * CR)])

    fin_wait(LAST, 0)
    fin_wait(LAST, 1)

    @pl.when(is0)
    def _():
        project(1, 1, [_unpack(rem[LAST]), _unpack(rem[NCH + LAST])])
        sent(own_sem, wqf.at[pl.ds(0, (NCH + 1) * CR)])
        sent(fw_sem, kf.at[pl.ds(0, 2 * LAST * CR)])
        sent(fw2_sem, kf.at[pl.ds(0, 2 * KEEP)])

    pl.when(me != 0)(lambda: project(1, 1, own_context(1, 1)))


def pallas_dist_sparse_attn_strided_qseq_kvseq_b2_sq128_skv128_hq4_dh64_kernel(
    x: jax.Array,
    Wq: jax.Array,
    K_ext: jax.Array,
    V_ext: jax.Array,
    Wo: jax.Array,
):
    kt = jnp.transpose(K_ext, (0, 2, 3, 1)).reshape(B * HD, S)
    vt = jnp.transpose(V_ext, (0, 2, 3, 1)).reshape(B * HD, S)
    vmem, dma = pltpu.VMEM, pltpu.SemaphoreType.DMA
    return pl.pallas_call(
        _body,
        out_shape=jax.ShapeDtypeStruct((B, S, DM), F32),
        in_specs=[pl.BlockSpec(memory_space=pl.ANY)] * 5,
        out_specs=pl.BlockSpec(memory_space=pltpu.VMEM),
        scratch_shapes=[
            vmem((B, S, DM), F32),
            vmem((DM, HD), F32),
            vmem((B * HD, S), F32),
            vmem((B * HD, S), F32),
            vmem((HD, DM), F32),
            vmem((2 * NCH, CR, 128), U32),
            vmem((2 * NCH, CR, 128), U32),
            vmem((2 * NRL, CR, 128), U32),
            vmem((DM // 2, HD), U32),
            vmem((HD // 2, DM), U32),
            vmem((8, BLK, 128), BF16),
            vmem((8, BLK, 128), F32),
            vmem((8, BLK, 128), BF16),
            vmem((8, BLK, 128), BF16),
            vmem((8, BLK, 128), F32),
            vmem((2, HEAD, 128), F32),
            vmem((BLK, 128), BF16),
            vmem((2, BLK, 128), BF16),
            vmem((BLK, 128), F32),
            vmem((CR, 128), U32),
            dma((2 * NPC + 14,)),
            dma,
            dma((2,)),
            dma,
            dma,
            dma((2 * NRL,)),
            dma((2 * NCH,)),
            dma((2,)),
            dma,
            pltpu.SemaphoreType.REGULAR,
        ],
        compiler_params=pltpu.CompilerParams(
            collective_id=0, disable_bounds_checks=True, disable_semaphore_checks=True),
    )(x, Wq, kt, vt, Wo)
```

```python
import jax
import jax.numpy as jnp
from jax import lax
from jax.experimental import pallas as pl
from jax.experimental.pallas import tpu as pltpu

B, S, DM, H, DH = 2, 128, 512, 4, 64
HD = H * DH
BLK = 64
F32, BF16, U32 = jnp.float32, jnp.bfloat16, jnp.uint32
MESH = pl.DeviceIdType.MESH
NT = (((1,), (1,)), ((), ()))
QSCALE = 0.125 * 1.4426950408889634

NCH = 8
LAST = NCH - 1
NRL = NCH + 1
CR = 32
HEAD_ODD = 22
HEAD_2 = 16
PC = 16
NPC = DH // PC - 1
SPLIT = 6
KEEP = 20


def _pack(x):
    return pltpu.bitcast(x.astype(BF16), U32)


def _unpack(w):
    return pltpu.bitcast(w, BF16)


def _body(x_hbm, wq_hbm, kt_hbm, vt_hbm, wo_hbm, out_ref,
          xf, wqf, kf, vf, wof, loc, rem, rl, wqb, wob, qb, sl, p_loc, p_rem, inv_l,
          hx, qx, px, inv_x, cx,
          ld_sem, own_sem, aux_sem, fw_sem, fw2_sem, rl_sem, fin_sem, hx_sem, qx_sem, rdy_sem):
    me = lax.axis_index("i")
    odd = me & 1
    nbr = (1 - odd, 3 - odd)
    side = me >> 1
    is0, is2, is_odd = me == 0, me == 2, odd == 1

    def signal(sem, dev):
        pl.semaphore_signal(sem, inc=1, device_id=(dev,), device_id_type=MESH)

    def rdma(src, dst, send_sem, recv_sem, dev):
        return pltpu.make_async_remote_copy(src, dst, send_sem, recv_sem,
                                            device_id=(dev,), device_id_type=MESH)

    bar = pltpu.get_barrier_semaphore()

    @pl.when(me != 2)
    def _():
        signal(bar, nbr[0])
        signal(bar, nbr[1])

    def head_send(p, n):
        return rdma(kt_hbm.at[pl.ds(p * 128, n)], hx.at[side, pl.ds(0, n)],
                    aux_sem.at[p], hx_sem.at[side], nbr[p])

    @pl.when(is_odd)
    def _():
        pl.semaphore_wait(bar, 1)
        head_send(0, HEAD_ODD).start()

    loads = []

    def load(src, dst):
        loads.append(pltpu.make_async_copy(src, dst, ld_sem.at[len(loads)]))
        return loads[-1]

    def load_rows(src, dst, r0, n):
        return load(src.at[pl.ds(r0, n)], dst.at[pl.ds(r0, n)])

    k0_tail = [[load_rows(kt_hbm, kf, p * 128 + PC * (j + 1), PC) for p in range(2)]
               for j in range(NPC)]
    k0_b = [load_rows(kt_hbm, kf, p * 128 + DH, DH) for p in range(2)]
    n_urgent = len(loads)
    k1 = [load_rows(kt_hbm, kf, HD + p * 128, 128) for p in range(2)]
    k0_head = [load_rows(kt_hbm, kf, p * 128, PC) for p in range(2)]
    v_ld = [[load_rows(vt_hbm, vf, b * HD + p * 128, 128) for b in range(B)] for p in range(2)]
    wq_ld = load(wq_hbm, wqf)
    x_ld = {b: load(x_hbm.at[b], xf.at[b]) for b in (1, 0)}
    wo_ld = load(wo_hbm, wof)

    for cp in loads[:n_urgent]:
        cp.start()

    @pl.when(is2)
    def _():
        pl.semaphore_wait(bar, 2)
        head_send(1, HEAD_2).start()
        head_send(0, HEAD_2).start()
        signal(rdy_sem, nbr[0])
        signal(rdy_sem, nbr[1])

    for cp in loads[n_urgent:]:
        cp.start()

    def own_send(c, p, via=None, slot=None, r0=0, n=CR):
        via = p if via is None else via
        slot = side * NRL + (c if slot is None else slot)
        rdma(loc.at[p * NCH + c, pl.ds(r0, n)], rl.at[slot, pl.ds(r0, n)],
             own_sem, rl_sem.at[slot], nbr[via]).start()

    def rl_wait(slot, s, r0=0, n=CR):
        ref = rl.at[s * NRL + slot, pl.ds(r0, n)]
        rdma(ref, ref, own_sem, rl_sem.at[s * NRL + slot], nbr[s]).wait_recv()

    def fwd(slot, s, dst=None, r0=0, n=CR):
        dst = side * NCH + slot if dst is None else dst
        rdma(rl.at[s * NRL + slot, pl.ds(r0, n)], rem.at[dst, pl.ds(r0, n)],
             fw_sem if n == CR else fw2_sem, fin_sem.at[dst], nbr[1 - s]).start()

    def relay(slot, s, dst=None, r0=0, n=CR):
        rl_wait(slot, s, r0, n)
        fwd(slot, s, dst, r0, n)

    def fin_wait(c, p):
        ref = rem.at[p * NCH + c]
        rdma(ref, ref, own_sem, fin_sem.at[p * NCH + c], nbr[p]).wait_recv()

    def sent(sem, ref):
        pltpu.make_async_copy(ref, ref, sem).wait()

    lo32 = lax.broadcasted_iota(jnp.int32, (CR, 128), 1) < BLK
    lo64 = lax.broadcasted_iota(jnp.int32, (BLK, 128), 1) < BLK
    row128 = lax.broadcasted_iota(jnp.int32, (128, 128), 0)
    col128 = lax.broadcasted_iota(jnp.int32, (128, 128), 1)

    def swap(t):
        return pltpu.roll(t, BLK, 1)

    def blocks(top, bot, flip=False):
        z = jnp.zeros_like(top)
        if flip:
            parts = [jnp.where(lo32, z, top), jnp.where(lo32, bot, z)]
        else:
            parts = [jnp.where(lo32, top, z), jnp.where(lo32, z, bot)]
        return _unpack(jnp.concatenate(parts, axis=0))

    def uid(b, blk, p):
        return (b * 2 + blk) * 2 + p

    def flipped(b, blk):
        return b == 0 and blk == 1

    def mm(a, w):
        return jnp.dot(a, w, preferred_element_type=F32)

    early = (me != 0, is2)

    for j in range(NPC):
        for p in range(2):
            k0_tail[j][p].wait()
            r0, r1 = PC * (j + 1), PC * (j + 2)
            loc[p * NCH, r0 // 2:r1 // 2, :] = _pack(kf[p * 128 + r0:p * 128 + r1, :])
            for who, head in ((is2, HEAD_2), (is_odd, HEAD_ODD))[:2 - p]:
                s0 = max(r0, head)
                pl.when(who)(lambda: own_send(0, p, r0=s0 // 2, n=(r1 - s0) // 2))

    for p in range(2):
        k0_b[p].wait()
        loc[p * NCH + 1] = _pack(kf[p * 128 + DH:(p + 1) * 128, :])
        pl.when(early[p])(lambda: own_send(1, p))

    for p in range(2):
        k1[p].wait()
        r = HD + p * 128
        a, b_ = _pack(kf[r:r + DH, :]), _pack(kf[r + DH:r + 128, :])
        cross = swap(jnp.where(lo32, b_, a))
        loc[p * NCH + 2] = jnp.where(lo32, a, cross)
        loc[p * NCH + 3] = jnp.where(lo32, cross, b_)

        @pl.when(early[p])
        def _():
            own_send(2, p)
            own_send(3, p)

    def prep_v(p):
        for b in range(B):
            v_ld[p][b].wait()
        eye = jnp.where(row128 == col128, 1.0, 0.0).astype(BF16)
        for b in range(B):
            r = b * HD + p * 128
            v = lax.dot_general(eye, vf[r:r + 128, :].astype(BF16), NT, preferred_element_type=F32)
            for blk in range(2):
                loc[p * NCH + 4 + 2 * b + blk] = _pack(v[blk * BLK:(blk + 1) * BLK])

    for p in range(2):
        k0_head[p].wait()
        loc[p * NCH, 0:PC // 2, :] = _pack(kf[p * 128:p * 128 + PC, :])
    prep_v(0)

    @pl.when(is2)
    def _():
        for c in range(4, NCH):
            own_send(c, 0)

    @pl.when(is_odd)
    def _():
        for c in range(4, NCH):
            own_send(c, 0, n=KEEP if c == SPLIT else CR)

    @pl.when(is0)
    def _():
        pl.semaphore_wait(bar, 2)
        for c in range(4):
            own_send(c, 0)
            own_send(c, 1)

    @pl.when(is_odd)
    def _():
        pl.semaphore_wait(rdy_sem, 1)
        for c in range(4):
            own_send(c, 1)

    prep_v(1)

    @pl.when(is2)
    def _():
        for c in range(4, NCH):
            own_send(c, 1)

    @pl.when(is_odd)
    def _():
        for c in range(4, NCH):
            if c == SPLIT:
                own_send(SPLIT, 0, via=1, slot=NCH, r0=KEEP, n=CR - KEEP)
            own_send(c, 1)

    def q_proj(b):
        x_ld[b].wait()
        q = mm(xf[b].astype(BF16), _unpack(wqb[...])) * QSCALE
        for blk in range(2):
            for p in range(2):
                qb[uid(b, blk, p)] = q[blk * BLK:(blk + 1) * BLK, p * 128:(p + 1) * 128].astype(BF16)

    def k_tile(buf, b, blk, p, swapped=True):
        c = p * NCH + 2 * b
        if b == 1:
            return blocks(buf[c + blk], buf[c + blk])
        return blocks(buf[c], buf[c + 1] if swapped else swap(buf[c + 1]), flipped(b, blk))

    def softmax(items):
        neg = jnp.float32(-jnp.inf)
        es = []
        for get_a, s_b, _ in items:
            mx = jnp.maximum(get_a(), s_b)
            m0 = jnp.max(jnp.where(lo64, mx, neg), axis=-1, keepdims=True)
            m1 = jnp.max(jnp.where(lo64, neg, mx), axis=-1, keepdims=True)
            m = jnp.where(lo64, m0, m1)
            es.append((jnp.exp2(get_a() - m), jnp.exp2(s_b - m)))
        res = []
        for (e_a, e_b), (_, _, flip) in zip(es, items):
            same = (row128 < BLK) == (col128 < BLK)
            ones = jnp.where(same != flip, 1.0, 0.0).astype(BF16)
            l = mm((e_a + e_b).astype(BF16), ones)
            r = pl.reciprocal(l, approx=True)
            res.append((e_a.astype(BF16), e_b.astype(BF16), r * (2.0 - l * r)))
        return res

    def context(p_a, v_a, p_b, v_b, inv, flip=False):
        return (mm(p_a, blocks(v_a, v_a, flip)) + mm(p_b, blocks(v_b, v_b, flip))) * inv

    wq_ld.wait()
    wqb[...] = _pack(wqf[...])
    q_proj(1)

    def q_send(p):
        return rdma(qb.at[uid(1, 1, p)], qx, aux_sem.at[p], qx_sem, nbr[p])

    @pl.when(is0)
    def _():
        for p in range(2):
            q_send(p).start()
        for c in (LAST, 4, 5, 6):
            own_send(c, 0)
            own_send(c, 1)

    def merge_head(s, n):
        ref = hx.at[s, pl.ds(0, n)]
        rdma(ref, ref, own_sem, hx_sem.at[s], nbr[s]).wait_recv()
        rl_wait(0, s, n // 2, CR - n // 2)
        rows = lax.broadcasted_iota(jnp.int32, (2 * PC, 128), 0)
        h = _pack(jnp.where(rows < n, hx[s], 0.0))
        top = lax.broadcasted_iota(jnp.int32, (PC, 128), 0) < n // 2
        rl[s * NRL, 0:PC, :] = jnp.where(top, h, rl[s * NRL, 0:PC, :])

    pl.when(is0)(lambda: merge_head(1, HEAD_ODD))
    pl.when(is_odd)(lambda: merge_head(1, HEAD_2))
    pl.when(is2)(lambda: rl_wait(0, 1))
    fwd(0, 1)
    pl.when(is0)(lambda: merge_head(0, HEAD_ODD))
    pl.when(me != 0)(lambda: rl_wait(0, 0))
    fwd(0, 0)

    for s in range(2):
        rl_wait(1, s)
    for s in range(2):
        rl[s * NRL + 1] = swap(rl[s * NRL + 1])
    for s in (1, 0):
        fwd(1, s)

    q_proj(0)
    relay(2, 1)
    relay(2, 0)
    for b in range(B):
        for p in range(2):
            for blk in range(2):
                sl[uid(b, blk, p)] = mm(qb[uid(b, blk, p)], k_tile(loc, b, blk, p, swapped=False))
    wo_ld.wait()
    wob[...] = _pack(wof[...])

    @pl.when(is0)
    def _():
        for slot in range(3, NCH):
            for s in range(2):
                relay(slot, s, n=KEEP if slot == SPLIT else CR)

    @pl.when(is2)
    def _():
        for slot in range(3, NCH):
            if slot == SPLIT:
                for s in range(2):
                    relay(NCH, s, dst=SPLIT, r0=KEEP, n=CR - KEEP)
            for s in range(2):
                relay(slot, s)

    @pl.when(is_odd)
    def _():
        relay(3, 0)
        rl_wait(3, 1)
        relay(4, 1)
        rdma(qx, qx, own_sem, qx_sem, nbr[0]).wait_recv()
        s_a = mm(qx[...], blocks(rl[3], rl[3]))
        s_b = mm(qx[...], blocks(rl[NRL + 3], rl[NRL + 3]))
        (px[0], px[1], inv_x[...]), = softmax([(lambda: s_a, s_b, False)])
        relay(5, 1)
        rl_wait(LAST, 0)
        relay(4, 0)
        relay(6, 1)
        relay(5, 0)
        rl_wait(LAST, 1)
        cx[...] = _pack(context(px[0], rl[LAST], px[1], rl[NRL + LAST], inv_x[...]))
        dst = side * NCH + LAST
        rdma(cx, rem.at[dst], fw_sem, fin_sem.at[dst], nbr[0]).start()
        relay(6, 0)
        fwd(LAST, 0)

    def scores(b, blks):
        units = [(blk, p) for blk in blks for p in range(2)]
        for blk, p in units:
            fin_wait(2 * b + blk, p)
        s_rem = [mm(qb[uid(b, blk, p)], k_tile(rem, b, blk, p)) for blk, p in units]
        res = softmax([(lambda u=uid(b, blk, p): sl[u], s, flipped(b, blk))
                       for (blk, p), s in zip(units, s_rem)])
        for (blk, p), r in zip(units, res):
            u = uid(b, blk, p)
            p_loc[u], p_rem[u], inv_l[u] = r

    scores(0, (0, 1))
    pl.when(is0)(lambda: scores(1, (0,)))
    pl.when(me != 0)(lambda: scores(1, (0, 1)))

    def project(b, blk, ctx):
        out_ref[b, blk * BLK:(blk + 1) * BLK, :] = (
            mm(ctx[0], _unpack(wob[0:DH, :])) + mm(ctx[1], _unpack(wob[DH:2 * DH, :])))

    def own_context(b, blk):
        res = []
        for p in range(2):
            u, c = uid(b, blk, p), p * NCH + 4 + 2 * b + blk
            res.append(context(p_loc[u], loc[c], p_rem[u], rem[c], inv_l[u],
                               flipped(b, blk)).astype(BF16))
        return res

    for c in range(4, LAST):
        fin_wait(c, 0)
        fin_wait(c, 1)
        project((c - 4) // 2, c % 2, own_context((c - 4) // 2, c % 2))

    @pl.when(is0)
    def _():
        sent(own_sem, kf)
        q_send(0).wait_send()
        q_send(1).wait_send()

    @pl.when(is2)
    def _():
        sent(own_sem, kf.at[pl.ds(0, 2 * NCH * CR - HEAD_2)])
        head_send(0, HEAD_2).wait_send()
        head_send(1, HEAD_2).wait_send()
        sent(fw_sem, kf)
        sent(fw2_sem, kf.at[pl.ds(0, 2 * (CR - KEEP))])

    @pl.when(is_odd)
    def _():
        sent(own_sem, kf.at[pl.ds(0, 2 * NCH * CR - HEAD_ODD // 2)])
        head_send(0, HEAD_ODD).wait_send()
        sent(fw_sem, kf.at[pl.ds(0, (2 * NCH - 1) * CR)])

    fin_wait(LAST, 0)
    fin_wait(LAST, 1)

    @pl.when(is0)
    def _():
        project(1, 1, [_unpack(rem[LAST]), _unpack(rem[NCH + LAST])])
        sent(fw_sem, kf.at[pl.ds(0, 2 * LAST * CR)])
        sent(fw2_sem, kf.at[pl.ds(0, 2 * KEEP)])

    pl.when(me != 0)(lambda: project(1, 1, own_context(1, 1)))


def pallas_dist_sparse_attn_strided_qseq_kvseq_b2_sq128_skv128_hq4_dh64_kernel(
    x: jax.Array,
    Wq: jax.Array,
    K_ext: jax.Array,
    V_ext: jax.Array,
    Wo: jax.Array,
):
    kt = jnp.transpose(K_ext, (0, 2, 3, 1)).reshape(B * HD, S)
    vt = jnp.transpose(V_ext, (0, 2, 3, 1)).reshape(B * HD, S)
    vmem, dma = pltpu.VMEM, pltpu.SemaphoreType.DMA
    return pl.pallas_call(
        _body,
        out_shape=jax.ShapeDtypeStruct((B, S, DM), F32),
        in_specs=[pl.BlockSpec(memory_space=pl.ANY)] * 5,
        out_specs=pl.BlockSpec(memory_space=pltpu.VMEM),
        scratch_shapes=[
            vmem((B, S, DM), F32),
            vmem((DM, HD), F32),
            vmem((B * HD, S), F32),
            vmem((B * HD, S), F32),
            vmem((HD, DM), F32),
            vmem((2 * NCH, CR, 128), U32),
            vmem((2 * NCH, CR, 128), U32),
            vmem((2 * NRL, CR, 128), U32),
            vmem((DM // 2, HD), U32),
            vmem((HD // 2, DM), U32),
            vmem((8, BLK, 128), BF16),
            vmem((8, BLK, 128), F32),
            vmem((8, BLK, 128), BF16),
            vmem((8, BLK, 128), BF16),
            vmem((8, BLK, 128), F32),
            vmem((2, 2 * PC, 128), F32),
            vmem((BLK, 128), BF16),
            vmem((2, BLK, 128), BF16),
            vmem((BLK, 128), F32),
            vmem((CR, 128), U32),
            dma((2 * NPC + 14,)),
            dma,
            dma((2,)),
            dma,
            dma,
            dma((2 * NRL,)),
            dma((2 * NCH,)),
            dma((2,)),
            dma,
            pltpu.SemaphoreType.REGULAR,
        ],
        compiler_params=pltpu.CompilerParams(
            collective_id=0, disable_semaphore_checks=True),
    )(x, Wq, kt, vt, Wo)
```
